```python
import numpy as np

kernel_name = "dist_argmax_global_i_m4096_n1024"

def setup_inputs():
    return {"x": np.random.randn(16384, 1024).astype(np.float32)}

def reference(x: np.ndarray) -> np.ndarray:
    idx = np.argmax(x, axis=0).astype(np.float32)
    val = np.max(x, axis=0)
    return np.stack([val, idx], axis=0)
```

```python
import jax
import jax.numpy as jnp
from jax import lax
from jax.experimental import pallas as pl
from jax.experimental.pallas import tpu as pltpu

N_DEV = 4
MESH = pl.DeviceIdType.MESH
SUB = 8
LANES = 128
NO_ROW = 1e9

PUSH = 216
BIG_CHUNKS = (2944, 400)
A_CHUNKS = (256, 64)
B_CHUNKS = (256, 64)
UNROLL = 8


def _starts(sizes):
    out, acc = [], 0
    for s in sizes:
        out.append(acc)
        acc += s
    return out


def _scan(ref, row0, nslab, cols, carry, slab0):
    lo = 0
    if carry is None:
        first = ref[pl.ds(row0, SUB), cols]
        carry = (first, jnp.full(first.shape, slab0, jnp.int32))
        lo = 1

    def step(s, carry):
        best, best_slab = carry
        v = ref[pl.ds(pl.multiple_of(row0 + s * SUB, SUB), SUB), cols]
        better = v > best
        return jnp.where(better, v, best), jnp.where(better, slab0 + s, best_slab)

    if nslab - lo <= UNROLL:
        for s in range(lo, nslab):
            carry = step(s, carry)
        return carry
    return lax.fori_loop(lo, nslab, step, carry, unroll=UNROLL)


def _tree(items):
    while len(items) > 1:
        merged = []
        for q in range(0, len(items) - 1, 2):
            (lv, li), (rv, ri) = items[q], items[q + 1]
            better = rv > lv
            merged.append((jnp.where(better, rv, lv), jnp.where(better, ri, li)))
        if len(items) % 2:
            merged.append(items[-1])
        items = merged
    return items[0]


def _rows(slab):
    sub = lax.broadcasted_iota(jnp.int32, slab.shape, 0)
    return (slab * SUB + sub).astype(jnp.float32)


def _reduce(best, best_slab, other):
    mx = jnp.maximum(jnp.max(best, axis=0, keepdims=True), other[0])
    row = jnp.min(jnp.where(best == mx, _rows(best_slab), NO_ROW), axis=0, keepdims=True)
    row = jnp.minimum(row, jnp.where(other[0] == mx, other[1], NO_ROW))
    return mx, row


def pallas_dist_argmax_global_i_m4096_n1024_kernel(x: jax.Array):
    m, n = x.shape
    n_local = m - 2 * PUSH
    tail = sum(A_CHUNKS)
    n_full = n_local - tail
    split = n - LANES
    assert sum(BIG_CHUNKS) == n_full and sum(B_CHUNKS) == tail
    assert all(s % SUB == 0 for s in (m, PUSH, *BIG_CHUNKS, *A_CHUNKS, *B_CHUNKS))
    assert n % LANES == 0 and split > 0
    n_big, n_a, n_b = len(BIG_CHUNKS), len(A_CHUNKS), len(B_CHUNKS)
    cols_a, cols_b = pl.ds(0, split), pl.ds(split, LANES)
    lanes_a, lanes_b = slice(0, split), slice(split, n)

    def kernel(x_hbm, out_ref, buf, theirs, parts, local_sems, push_sems, send_sems,
               theirs_sem, parts_sem):
        me = lax.axis_index("i")

        def peer(k):
            return (me + k) % N_DEV

        def local_copy(i, rows, cols):
            return pltpu.make_async_copy(
                x_hbm.at[rows, cols], buf.at[rows, cols], local_sems.at[i])

        big = [local_copy(j, pl.ds(r0, nr), pl.ds(0, n))
               for j, (r0, nr) in enumerate(zip(_starts(BIG_CHUNKS), BIG_CHUNKS))]
        part_a = [local_copy(n_big + j, pl.ds(n_full + r0, nr), cols_a)
                  for j, (r0, nr) in enumerate(zip(_starts(A_CHUNKS), A_CHUNKS))]
        part_b = [local_copy(n_big + n_a + j, pl.ds(n_full + r0, nr), cols_b)
                  for j, (r0, nr) in enumerate(zip(_starts(B_CHUNKS), B_CHUNKS))]
        for copy in big + part_a + part_b:
            copy.start()

        barrier = pltpu.get_barrier_semaphore()
        for k in (2, 1, 3):
            pl.semaphore_signal(barrier, inc=1, device_id=(peer(k),), device_id_type=MESH)
        pl.semaphore_wait(barrier, N_DEV - 1)

        pushes = []
        for slot, k in enumerate((1, 3)):
            push = pltpu.make_async_remote_copy(
                src_ref=x_hbm.at[pl.ds(n_local + slot * PUSH, PUSH)],
                dst_ref=theirs.at[slot],
                send_sem=push_sems.at[slot], recv_sem=theirs_sem,
                device_id=(peer(k),), device_id_type=MESH)
            push.start()
            pushes.append(push)

        my_slab0 = me * (m // SUB)
        best = None
        for copy, r0, nr in zip(big, _starts(BIG_CHUNKS), BIG_CHUNKS):
            copy.wait()
            best = _scan(buf, r0, nr // SUB, slice(None), best, my_slab0 + r0 // SUB)

        pltpu.make_async_copy(theirs, theirs, theirs_sem).wait()
        v0, s0 = _scan(theirs.at[0], 0, PUSH // SUB, slice(None), None,
                       peer(3) * (m // SUB) + n_local // SUB)
        v1, s1 = _scan(theirs.at[1], 0, PUSH // SUB, slice(None), None,
                       peer(1) * (m // SUB) + (n_local + PUSH) // SUB)
        side_max = jnp.max(jnp.maximum(v0, v1), axis=0, keepdims=True)
        side_row = jnp.min(
            jnp.minimum(jnp.where(v0 == side_max, _rows(s0), NO_ROW),
                        jnp.where(v1 == side_max, _rows(s1), NO_ROW)),
            axis=0, keepdims=True)

        sends = []

        def send(k, cols):
            copy = pltpu.make_async_remote_copy(
                src_ref=parts.at[0, :, cols], dst_ref=parts.at[k, :, cols],
                send_sem=send_sems.at[len(sends)], recv_sem=parts_sem,
                device_id=(peer(k),), device_id_type=MESH)
            copy.start()
            sends.append(copy)

        best_a = (best[0][:, lanes_a], best[1][:, lanes_a])
        for copy, r0, nr in zip(part_a, _starts(A_CHUNKS), A_CHUNKS):
            copy.wait()
            row0 = n_full + r0
            best_a = _scan(buf, row0, nr // SUB, cols_a, best_a, my_slab0 + row0 // SUB)
        parts[0, :, cols_a] = jnp.concatenate(
            _reduce(*best_a, (side_max[:, lanes_a], side_row[:, lanes_a])), axis=0)
        send(2, cols_a)

        best_b = (best[0][:, lanes_b], best[1][:, lanes_b])
        other = (side_max[:, lanes_b], side_row[:, lanes_b])
        for j, (copy, r0, nr) in enumerate(zip(part_b, _starts(B_CHUNKS), B_CHUNKS)):
            last = j == n_b - 1
            if last:
                other = _reduce(*best_b, other)
            copy.wait()
            row0 = n_full + r0
            slabs = [(buf[pl.ds(row0 + SUB * s, SUB), cols_b],
                      jnp.full((SUB, LANES), my_slab0 + row0 // SUB + s, jnp.int32))
                     for s in range(nr // SUB)]
            best_b = _tree(slabs if last else [best_b] + slabs)
        parts[0, :, cols_b] = jnp.concatenate(_reduce(*best_b, other), axis=0)
        send(2, cols_b)
        for cols in (cols_a, cols_b):
            send(1, cols)
            send(3, cols)

        for copy in pushes + sends:
            copy.wait_send()
        received = parts.at[pl.ds(1, N_DEV - 1)]
        pltpu.make_async_copy(received, received, parts_sem).wait()

        vals = [parts[k, 0:1, :] for k in range(N_DEV)]
        rows = [parts[k, 1:2, :] for k in range(N_DEV)]
        gmax = jnp.maximum(jnp.maximum(vals[0], vals[1]), jnp.maximum(vals[2], vals[3]))
        cand = [jnp.where(v == gmax, r, NO_ROW) for v, r in zip(vals, rows)]
        out_ref[0:1, :] = gmax
        out_ref[1:2, :] = jnp.minimum(jnp.minimum(cand[0], cand[1]),
                                      jnp.minimum(cand[2], cand[3]))

    return pl.pallas_call(
        kernel,
        out_shape=jax.ShapeDtypeStruct((2, n), jnp.float32),
        in_specs=[pl.BlockSpec(memory_space=pl.ANY)],
        out_specs=pl.BlockSpec(memory_space=pltpu.VMEM),
        scratch_shapes=[
            pltpu.VMEM((n_local, n), jnp.float32),
            pltpu.VMEM((2, PUSH, n), jnp.float32),
            pltpu.VMEM((N_DEV, 2, n), jnp.float32),
            pltpu.SemaphoreType.DMA((n_big + n_a + n_b,)),
            pltpu.SemaphoreType.DMA((2,)),
            pltpu.SemaphoreType.DMA((2 * (N_DEV - 1),)),
            pltpu.SemaphoreType.DMA,
            pltpu.SemaphoreType.DMA,
        ],
        compiler_params=pltpu.CompilerParams(
            collective_id=0,
            vmem_limit_bytes=32 * 1024 * 1024,
            disable_semaphore_checks=True,
        ),
    )(x)
```
